```python
import numpy as np

kernel_name = "dist_moe_cap_ep_tokshard_n2048_d512_e8_h1024"

def setup_inputs():
    x = np.random.randn(8192, 512).astype(np.float32)
    router_W = np.random.randn(512, 32).astype(np.float32) * 0.1
    scores64 = x.astype(np.float64) @ router_W.astype(np.float64)
    route_idx = np.argsort(-scores64, axis=-1)[:, :1].astype(np.int32)
    expert_W = np.random.randn(32, 512, 1024).astype(np.float32) * 0.02
    return {"x": x, "router_W": router_W, "route_idx": route_idx, "expert_W": expert_W}

def reference(x, router_W, route_idx, expert_W):
    counts = np.zeros(32, dtype=np.int64)
    out = np.zeros((8192, 1024), dtype=np.float32)
    for i in range(8192):
        e = int(route_idx[i, 0])
        if counts[e] < 204:
            out[i] = x[i] @ expert_W[e]
            counts[e] += 1
    return out
```

```python
import contextlib

import jax
import jax.numpy as jnp
from jax import lax
from jax.experimental import pallas as pl
from jax.experimental.pallas import tpu as pltpu

NDEV = 4
NT = 2048
D = 512
H = 1024
NE = 32
EL = 8
CAP = 204
ROWS = 16
MROWS = 208

CD_SH = 5
CC_SH = 3
CD, CC = 1 << CD_SH, 1 << CC_SH
CHD, CHC = 2 * CD, 4 * CC
KD, KC = (CD_SH, 2, CHD), (CC_SH, 1, CHC)

SR = 3
DOFF = (0, SR * 128 + CD)
REGD = NT + 2 * CD
ND0 = SR * 128 // CD
NDSEM = 3 * ND0 + EL * CAP // CD + NDEV
REGC = 1664
NCSEM = NT // CC + NDEV
NRELAY = 768 // (2 * CC)

OVER = 3
A_EARLY = 5
NLIST = A_EARLY * CAP // CC + 8
CGROUPS = (0, 4, 7, 10, 12, 13, 14, 15, 16)
START = (140, 150, 175, 150)
FIRSTC = 590
YIDLE = 260
LIGHT = 450
CREDIT = 5
MID = 5
SPARE = 2
LEAD = 4
DEAD = (80, 0, 0, 0)
NPRE = 7
TAIL_A = (0, 0, 6, 0)
TAIL_B = (0, 0, 0, 3)
DRAIN = (140, 160, 180, 200, 215, 228, 238, 245)

ZROWS = MROWS + 16
TROWS = 80

PROFILE_SCOPES = False


def _scope(name):
    if PROFILE_SCOPES:
        return jax.named_scope(name)
    return contextlib.nullcontext()


def _iota(shape, dim):
    return lax.broadcasted_iota(jnp.int32, shape, dim)


def _group_bound(r, groups, end):
    out = jnp.full(r.shape, groups[1] if end else groups[0], jnp.int32)
    for g in range(1, len(groups) - 1):
        out = jnp.where(r >= groups[g], groups[g + 1] if end else groups[g], out)
    return out


def _bf(x):
    return x.astype(jnp.bfloat16)


def _one(mask):
    return _bf(jnp.where(mask, 1.0, 0.0))


def _dot(a, b):
    return jnp.dot(a, b, preferred_element_type=jnp.float32)


def _pack(lo, hi):
    lo_b = lax.bitcast_convert_type(_bf(lo).astype(jnp.float32), jnp.uint32)
    hi_b = lax.bitcast_convert_type(_bf(hi).astype(jnp.float32), jnp.uint32)
    return (lo_b >> 16) | hi_b


def _unpack_lo(v):
    return lax.bitcast_convert_type(v << 16, jnp.float32)


def _unpack_hi(v):
    return lax.bitcast_convert_type(v & jnp.uint32(0xFFFF0000), jnp.float32)


def _split(v):
    hi = jnp.floor(v * (1.0 / 128.0))
    return hi, v - 128.0 * hi


def _body(x_hbm, r_hbm, w_hbm, o_ref,
          xf, rv, wf, cntb, tabv, s0v, slotv, R, XB, L, Z, YB,
          tabs, s0s, slots, st, lst,
          lsem, cnt_sem, dsem, csem, rsem, ssem):
    me = lax.axis_index("i")
    MESH = pl.DeviceIdType.MESH
    peers = [me ^ k for k in range(NDEV)]
    order = (2, 1, 3)

    r_cp = pltpu.make_async_copy(r_hbm, rv, lsem.at[0])
    r_cp.start()

    bar = pltpu.get_barrier_semaphore()
    for k in order:
        pl.semaphore_signal(bar, inc=1, device_id=(peers[k],), device_id_type=MESH)

    def x_cp(row):
        sl = pl.ds(pl.multiple_of(row * 128, 128), 128)
        return pltpu.make_async_copy(x_hbm.at[sl], xf.at[sl], lsem.at[16 + row])

    for row in range(ROWS):
        x_cp(row).start()

    def w_cp(j):
        return pltpu.make_async_copy(w_hbm.at[j], wf.at[j], lsem.at[8 + j])

    for j in range(EL):
        w_cp(j).start()

    YB[pl.ds(pl.multiple_of(me * (REGC * 4), 8), 8), :] = jnp.zeros((8, 128), jnp.uint32)

    with _scope("spec"):
        ur, uc = _iota((128, 256), 0), _iota((128, 256), 1)
        u2 = _one(ur < uc)
        qs, ql = _iota((128, 128), 0), _iota((128, 128), 1)
        e1, e2 = qs & 31, ql & 31
        diag = e1 == e2
        lt_same = (e1 < e2) & ((e1 >> 3) == (e2 >> 3))
        tabm = (ql == e1) | (ql == NE + (e1 >> 3))
        mprec = _one((ql < SR * NE) & (((e2 < e1) & ((e1 >> 3) == (e2 >> 3)))
                                       | (diag & (ql < qs))))
        a1 = _one(_iota((8, 128), 1) < SR * NE)
        r8 = _iota((8, 128), 0)
        e_io = _iota((NE, 128), 0)
        r_cp.wait()
        route = rv[...]

        def onehot(r0, r1):
            return jnp.concatenate(
                [jnp.where(route[r:r + 1, :] == e_io, 1.0, 0.0) for r in range(r0, r1)],
                axis=0)

        oh_a = onehot(0, 4)
        pt_a = _dot(_bf(oh_a), u2)
        tot_a = pt_a[:, 128:]
        val = oh_a * (_dot(mprec, _bf(tot_a)) + pt_a[:, :128])
        tabrow = _dot(a1, _bf(jnp.where(tabm, tot_a, 0.0)))
        pos0 = jnp.zeros((8, 128), jnp.float32)
        for r in range(SR):
            pos0 = jnp.where(r8 == r, jnp.sum(val[r * NE:(r + 1) * NE], axis=0,
                                              keepdims=True), pos0)
        dst = route >> 3
        dreg = jnp.where(dst == me, NDEV + me, dst) * REGD
        valid0 = (route[0:8] >= 0) & (route[0:8] < NE)
        s0 = jnp.where(valid0, dreg[0:8] + pos0.astype(jnp.int32), me * REGD) * 2
        s0v[...] = jnp.where(r8 < SR, s0, tabrow.astype(jnp.int32))
        s0_cp = pltpu.make_async_copy(s0v, s0s, lsem.at[1])
        s0_cp.start()

    with _scope("hist"):
        blk = _one((_iota((ROWS, 512), 1) >> 5) == _iota((ROWS, 512), 0))
        oh_b = onehot(4, ROWS)
        pt = jnp.concatenate([pt_a, _dot(_bf(oh_b), u2)], axis=0)
        oh_f = jnp.concatenate([oh_a, oh_b], axis=0)
        oh = _bf(oh_f)
        pre, tot = pt[:, :128], pt[:, 128:]
        totd = jnp.concatenate(
            [jnp.where(diag, tot[i * 128:(i + 1) * 128], 0.0) for i in range(4)], axis=0)
        ic = _dot(blk, jnp.concatenate([_bf(oh_f * pre), _bf(totd)], axis=1))
        inrow = ic[:, :128]
        my_rows = pl.ds(pl.multiple_of(me * ROWS, ROWS), ROWS)
        cntb[my_rows, :] = ic[:, 128:]

    def cnt_cp(k):
        return pltpu.make_async_remote_copy(
            src_ref=cntb.at[my_rows], dst_ref=cntb.at[my_rows],
            send_sem=cnt_sem.at[3 + k - 1], recv_sem=cnt_sem.at[k - 1],
            device_id=(peers[k],), device_id_type=MESH)

    def load_pack(row):
        with _scope("xwait"):
            x_cp(row).wait()
        with _scope("pack"):
            for b in range(2):
                r0 = pl.multiple_of(row * 128 + b * 64, 64)
                xa = xf[pl.ds(r0, 64), :]
                for c in range(2):
                    R[pl.ds(2 * r0 + c, 64, stride=2), :] = _pack(
                        xa[:, c * 128:(c + 1) * 128],
                        xa[:, 256 + c * 128:256 + (c + 1) * 128])

    def permute_row(tbl, row):
        with _scope("permute"):
            src0 = row * 256
            for k in range(128):
                s = tbl[row, k]
                XB[pl.ds(s, 2), :] = R[pl.ds(src0 + 2 * k, 2), :]

    def d_send(k, g, c, nsub):
        dev = peers[k]
        soff = pl.multiple_of((dev * REGD + DOFF[g]) * 2 + c * CHD, 8)
        doff = pl.multiple_of(((NDEV + me) * REGD + DOFF[g]) * 2 + c * CHD, 8)
        sem0 = (k - 1) * ND0 if g == 0 else st[ST_DO + k]
        return pltpu.make_async_remote_copy(
            src_ref=XB.at[pl.ds(soff, nsub)], dst_ref=XB.at[pl.ds(doff, nsub)],
            send_sem=ssem.at[0], recv_sem=dsem.at[sem0 + c],
            device_id=(dev,), device_id_type=MESH)

    def d_recv(s, g, c, nsub):
        off = pl.multiple_of(((NDEV + s) * REGD + DOFF[g]) * 2 + c * CHD, 8)
        ref = XB.at[pl.ds(off, nsub)]
        sem0 = ((me ^ s) - 1) * ND0 if g == 0 else st[ST_DI + s]
        return pltpu.make_async_remote_copy(
            src_ref=ref, dst_ref=ref, send_sem=ssem.at[0],
            recv_sem=dsem.at[sem0 + c],
            device_id=(s,), device_id_type=MESH)

    def partial(tot_, kind, fn):
        sh, tsh, chsub = kind
        ntiles = ((tot_ & ((1 << sh) - 1)) + (1 << tsh) - 1) >> tsh
        for v in range(1, chsub // 8 + 1):
            @pl.when(ntiles == v)
            def _():
                fn(v * 8)

    def advance(idx, need, tot_, kind, fn):
        done = st[idx]

        @pl.when(need > done)
        def _():
            nfull = tot_ >> kind[0]

            def b(c, _):
                fn(c, kind[2])
                return 0

            lax.fori_loop(done, jnp.minimum(need, nfull), b, 0)

            @pl.when(need > nfull)
            def _():
                partial(tot_, kind, lambda n: fn(nfull, n))

            st[idx] = need

    def nchunks(tot_, sh):
        return (tot_ + (1 << sh) - 1) >> sh

    ST_X = 0
    ST_PS = 12
    ST_DW = 16
    ST_DP = 24
    ST_WP = 32
    ST_CS = 36
    ST_PG = 40
    ST_CO = 44
    ST_RO = 48
    ST_NR = 52
    ST_SW = 60
    ST_CG = 64
    ST_NE = 84
    ST_ND = 96
    ST_DO = 144
    ST_DI = 148
    for i in range(12, 44):
        st[i] = 0
    lst[NLIST] = 0
    for i, b_ in enumerate(CGROUPS):
        st[ST_CG + i] = b_

    def enter():
        with _scope("barrier"):
            pl.semaphore_wait(bar, NDEV - 1)
        for k in order:
            cnt_cp(k).start()

    @pl.when(me != 0)
    def _():
        enter()

    def row0(row, _):
        load_pack(row)

        @pl.when(row == 0)
        def _():
            s0_cp.wait()

        permute_row(s0s, row)
        return 0

    lax.fori_loop(0, SR, row0, 0)

    @pl.when(me == 0)
    def _():
        enter()

    def send_dispatch(g, tots, delay2):
        nfull = [None] + [tots[k] >> CD_SH for k in range(1, NDEV)]

        def sb(i, _):
            for k in order:
                c = i - delay2 if k == 2 else i

                @pl.when((c >= 0) & (c < nfull[k]))
                def _():
                    d_send(k, g, c, CHD).start()

                @pl.when(c == nfull[k])
                def _():
                    partial(tots[k], KD, lambda n: d_send(k, g, c, n).start())
            return 0

        nmax = jnp.maximum(jnp.maximum(nfull[1], nfull[2] + delay2), nfull[3])
        lax.fori_loop(0, nmax + 1, sb, 0)

    with _scope("phaseA"):
        s0row = s0s.at[SR]
        send_dispatch(0, [None] + [s0row[NE + peers[k]] for k in range(1, NDEV)], 0)

    with _scope("consts"):
        NSEL = 6 * ROWS
        sr = _iota((NSEL, 64), 0)
        rr = sr & 15
        sec = sr >> 4
        thr = rr
        thr = jnp.where(sec == 1, SR, thr)
        thr = jnp.where(sec == 2, _group_bound(rr, CGROUPS, False), thr)
        thr = jnp.where(sec == 3, _group_bound(rr, CGROUPS, True), thr)
        thr = jnp.where(sec == 4, 0, thr)
        thr = jnp.where(sec == 5, ROWS, thr)
        lsel = _one(_iota((NSEL, 64), 1) < thr + me * ROWS)
        lall = _one(_iota((72, 64), 1) < _iota((72, 64), 0))
        lr_, lc_ = _iota((8, 64), 0), _iota((8, 64), 1)
        lraw = _one(((lc_ >> 4) == lr_) & ((lc_ & 15) < SR))
        q = qs >> 5
        same = (e1 >> 3) == (e2 >> 3)
        late1 = (e1 & 7) >= A_EARLY
        late12 = late1 & ((e2 & 7) >= A_EARLY)
        c_sel = (((q == 1) & lt_same & jnp.logical_not(late1))
                 | ((q == 2) & same & late12) | ((q == 3) & lt_same & late12))
        mbase = jnp.concatenate([_one((q == 0) & lt_same), _one(c_sel)], axis=1)
        mtab = _one((qs < NE) & (tabm | ((ql == NE + NDEV + (e1 >> 3)) & late1)))

    def pre(row, _):
        load_pack(row)
        return 0

    lax.fori_loop(SR, NPRE, pre, 0)

    with _scope("cntwait"):
        for k in range(1, NDEV):
            src_dev = peers[k]
            rows_k = cntb.at[pl.ds(pl.multiple_of(src_dev * ROWS, ROWS), ROWS)]
            pltpu.make_async_remote_copy(
                src_ref=rows_k, dst_ref=rows_k,
                send_sem=cnt_sem.at[3 + k - 1], recv_sem=cnt_sem.at[k - 1],
                device_id=(src_dev,), device_id_type=MESH).wait_recv()

    with _scope("slots"):
        cnt_all = _bf(cntb[...])
        gk = jnp.minimum(_dot(lsel, cnt_all), float(CAP))
        gA, gS, gD, gE, gF, gG = [gk[i * ROWS:(i + 1) * ROWS] for i in range(6)]
        lane = _iota((ROWS, 128), 1)
        quarter = lane >> 5
        lhs1 = jnp.where(quarter == 0, gG - gS,
                         jnp.where(quarter == 1, gG - gF,
                                   jnp.where(quarter == 2, gD - gF, gE - gD)))
        bases = _dot(_bf(lhs1), mbase)
        late_l = (lane & 7) >= A_EARLY
        dbase = jnp.maximum(bases[:, :128] + (gA - gS), 0.0)
        cbase = bases[:, 128:] + jnp.where(late_l, gA - gD, gA - gF)
        rem = float(CAP) - gA
        tables = [rem, *_split(dbase), *_split(cbase)]
        srow = _iota((ROWS, 128), 0)
        look_l = jnp.concatenate(
            [jnp.concatenate([jnp.where(srow == 4 * t + quarter, tb, 0.0) for t in range(4)],
                             axis=1) for tb in tables], axis=0)
        look = _dot(_bf(look_l), oh)
        kept = inrow < look[0:16]
        dpos = (look[16:32] * 128.0 + look[32:48] + inrow).astype(jnp.int32)
        cpos = (look[48:64] * 128.0 + look[64:80] + inrow).astype(jnp.int32)
        slotv[0:ROWS, :] = jnp.where(kept, dreg + DOFF[1] + dpos, me * REGD) * 2
        s_cp = pltpu.make_async_copy(slotv.at[pl.ds(0, ROWS)], slots.at[pl.ds(0, ROWS)],
                                     lsem.at[2])
        s_cp.start()
        gall = jnp.minimum(_dot(lall, cnt_all), float(CAP))
        tabv[0:72, :] = _dot(_bf(gall), mtab).astype(jnp.int32)
        tabv[72:80, :] = _dot(lraw, _bf(_dot(cnt_all, mtab))).astype(jnp.int32)
        t_cp = pltpu.make_async_copy(tabv, tabs, lsem.at[3])
        t_cp.start()
        slotv[ROWS:2 * ROWS, :] = jnp.where(kept, (NDEV + dst) * REGC + cpos, me * REGC) * 4
        c_cp = pltpu.make_async_copy(slotv.at[pl.ds(ROWS, ROWS)],
                                     slots.at[pl.ds(ROWS, ROWS)], lsem.at[4])
        c_cp.start()

    def T(row, lane_):
        return tabs.at[row][lane_]

    def kept_between(s, ra, rb, lane_):
        return T(s * ROWS + rb, lane_) - T(s * ROWS + ra, lane_)

    def slen(s, d):
        return kept_between(s, 0, ROWS, NE + d)

    def dlen(s, g, lane_):
        if g == 0:
            return T(72 + s, lane_)
        return kept_between(s, SR, ROWS, lane_)

    def dsem_off(s, d):
        off = 3 * ND0
        for ss in range(NDEV - 1):
            off = off + jnp.where((ss < s) & (ss != d),
                                  nchunks(dlen(ss, 1, NE + d), CD_SH), 0)
        return off

    def is_light(s):
        xl = 0
        for g in range(2):
            xl = xl + dlen(s, g, NE + (s ^ 3)) + dlen(s, g, NE + (s ^ 2))
        return xl < LIGHT

    def csem_off(s, d):
        off = 0
        for dd in range(NDEV - 1):
            off = off + jnp.where((dd < d) & (dd != s), nchunks(slen(s, dd), CC_SH), 0)
        return off

    def lists(s, r_off, d_off):
        ne, nr = st[ST_NE + s], st[ST_NR + s]

        def lb(c, carry):
            acc, i = carry
            acc = acc + nr
            hit = acc >= ne
            lst[jnp.where(hit, r_off + i, d_off + c - i)] = c
            return (jnp.where(hit, acc - ne, acc), i + hit.astype(jnp.int32))

        lax.fori_loop(0, ne, lb, (jnp.int32(0), jnp.int32(0)))

    def plan():
        for s in range(NDEV):
            st[ST_DI + s] = dsem_off(s, me)
        for i in range(1, NDEV):
            st[ST_CO + i] = csem_off(peers[i], me)
            st[ST_RO + i] = csem_off(me, peers[i])

        dmat = [[dlen(s, 0, NE + d) + dlen(s, 1, NE + d) for d in range(NDEV)]
                for s in range(NDEV)]
        kmat = [[slen(s, d) for d in range(NDEV)] for s in range(NDEV)]
        disp, comb = {}, {}
        for s in range(NDEV):
            for d in (s ^ 1, 3 - s):
                disp[(s, d)] = dmat[s][d]
                comb[(s, d)] = 2 * kmat[d][s]
        for s in range(NDEV):
            d, via = s ^ 2, 3 - s
            for lk_ in ((s, via), (via, d)):
                disp[lk_] = disp[lk_] + dmat[s][d]
                comb[lk_] = comb[lk_] + 2 * kmat[d][s]
        links = sorted(disp)
        load = {lk_: comb[lk_] + jnp.maximum(disp[lk_] + START[lk_[0]], FIRSTC)
                for lk_ in links}
        for s in range(NDEV):
            load[(s, s ^ 1)] = (load[(s, s ^ 1)] + DEAD[s ^ 1]
                                + jnp.maximum(YIDLE - dmat[s][s ^ 1], 0))
        theta = 0
        for l1, l2 in (((2, 1), (3, 0)), ((1, 0), (2, 3)), ((0, 3), (1, 2)),
                       ((3, 2), (0, 1))):
            theta = jnp.maximum(theta, (load[l1] + load[l2]) >> 1)
        cap = []
        for s in range(NDEV):
            ne = (kmat[s ^ 2][s] - kept_between(s ^ 2, 0, ROWS, NE + NDEV + s)) >> CC_SH
            st[ST_NE + s] = ne
            cap.append(jnp.minimum(ne, NRELAY))

        def sq(v):
            v = jnp.maximum(v, 0)
            return v * v

        def descend(it, carry):
            ex = dict(zip(links, carry[:8]))
            nrel = list(carry[8:])
            step = 16 >> (it >> 1)
            kib = step * (2 * CC)
            for s in (2, 3, 0, 1):
                dflt = ((s, 3 - s), (3 - s, s ^ 2))
                alt = ((s, s ^ 1), (s ^ 1, s ^ 2))
                cur = sum(sq(ex[l]) for l in dflt + alt)
                up = sum(sq(ex[l] - kib) for l in dflt) + sum(sq(ex[l] + kib) for l in alt)
                dn = sum(sq(ex[l] + kib) for l in dflt) + sum(sq(ex[l] - kib) for l in alt)
                sgn = jnp.where((up < cur) & (nrel[s] + step <= cap[s]), 1,
                                jnp.where((dn < cur) & (nrel[s] >= step), -1, 0))
                nrel[s] = nrel[s] + sgn * step
                for l in dflt:
                    ex[l] = ex[l] - sgn * kib
                for l in alt:
                    ex[l] = ex[l] + sgn * kib
            return tuple(ex[l] for l in links) + tuple(nrel)

        zero = jnp.int32(0)
        res = lax.fori_loop(0, 10, descend,
                            tuple(load[l] - theta for l in links) + (zero,) * NDEV)
        for s in range(NDEV):
            st[ST_NR + s] = res[8 + s]
        st[ST_NR + NDEV] = csem_off(3 - me, me ^ 1)
        nr_in, nr_out = st[ST_NR + (me ^ 1)], st[ST_NR + me]

        lists(me, 0, NLIST)

        n_ae = (slen(peers[3], me)
                - kept_between(peers[3], 0, ROWS, NE + NDEV + me)) >> CC_SH
        n_be = st[ST_NE + me] - nr_out
        n_al = (slen(peers[3], me) >> CC_SH) - n_ae
        n_bl = (slen(peers[2], me) >> CC_SH) - st[ST_NE + me]
        hold = jnp.clip(n_bl + pick(TAIL_A) + SPARE - n_al - nr_in, 0,
                        jnp.maximum(n_ae - n_be, 0))
        st[ST_X + 1] = n_ae - hold
        late_x = (n_be + n_bl > n_ae + n_al + nr_in).astype(jnp.int32)
        st[ST_X + 5] = n_be - late_x * jnp.minimum(n_al + nr_in, n_be >> 1)
        st[ST_X + 10] = late_x
        set_ratio(n_ae - hold + jnp.clip(n_be - n_ae, 0, nr_in), n_be)
        st[ST_X + 6] = 0
        st[ST_X + 0] = 0
        st[ST_X + 7] = n_ae
        st[ST_X + 8] = nr_in

    def pick(tbl):
        return jnp.where(me == 0, tbl[0], jnp.where(
            me == 1, tbl[1], jnp.where(me == 2, tbl[2], tbl[3])))

    def set_ratio(na, nb):
        aeff, beff = jnp.maximum(na, 1), jnp.maximum(nb, 1)
        rich = beff > aeff
        st[ST_X + 2] = jnp.where(rich, 1, aeff)
        st[ST_X + 3] = jnp.where(rich, 1, beff)
        st[ST_X + 9] = rich.astype(jnp.int32)
        st[ST_X + 4] = 0

    def row1(row, _):
        @pl.when(row >= NPRE)
        def _():
            load_pack(row)

        @pl.when(row == SR)
        def _():
            with _scope("slotwait"):
                s_cp.wait()

        permute_row(slots, row)
        return 0

    lax.fori_loop(SR, ROWS, row1, 0)
    with _scope("phaseB"):
        t_cp.wait()
        for k in range(1, NDEV):
            st[ST_DO + k] = dsem_off(me, peers[k])
        send_dispatch(1, [None] + [dlen(me, 1, NE + peers[k]) for k in range(1, NDEV)],
                      jnp.where(is_light(peers[3]), jnp.minimum(nchunks(
                          dlen(me, 1, peers[3] * EL) + OVER, CD_SH), LEAD), 0))
    light = is_light(me)
    with _scope("plan"):
        plan()

    def c_send(k, c, nsub):
        dev = peers[k]
        soff = pl.multiple_of(dev * (REGC * 4) + c * CHC, 8)
        doff = pl.multiple_of((NDEV + me) * (REGC * 4) + c * CHC, 8)
        return pltpu.make_async_remote_copy(
            src_ref=YB.at[pl.ds(soff, nsub)], dst_ref=YB.at[pl.ds(doff, nsub)],
            send_sem=ssem.at[1], recv_sem=csem.at[st[ST_CO + k] + c],
            device_id=(dev,), device_id_type=MESH)

    def c_recv(k, c, nsub):
        dev = peers[k]
        off = pl.multiple_of((NDEV + dev) * (REGC * 4) + c * CHC, 8)
        ref = YB.at[pl.ds(off, nsub)]
        return pltpu.make_async_remote_copy(
            src_ref=ref, dst_ref=ref, send_sem=ssem.at[1],
            recv_sem=csem.at[st[ST_RO + k] + c],
            device_id=(dev,), device_id_type=MESH)

    def relay1(c, i):
        soff = pl.multiple_of(peers[2] * (REGC * 4) + c * CHC, 8)
        doff = pl.multiple_of(peers[1] * (REGC * 4) + (i + 1) * CHC, 8)
        return pltpu.make_async_remote_copy(
            src_ref=YB.at[pl.ds(soff, CHC)], dst_ref=YB.at[pl.ds(doff, CHC)],
            send_sem=ssem.at[1], recv_sem=rsem.at[i],
            device_id=(peers[1],), device_id_type=MESH)

    def relay2(c, i):
        soff = pl.multiple_of(me * (REGC * 4) + (i + 1) * CHC, 8)
        doff = pl.multiple_of((NDEV + peers[1]) * (REGC * 4) + c * CHC, 8)
        return pltpu.make_async_remote_copy(
            src_ref=YB.at[pl.ds(soff, CHC)], dst_ref=YB.at[pl.ds(doff, CHC)],
            send_sem=ssem.at[1], recv_sem=csem.at[st[ST_NR + NDEV] + c],
            device_id=(peers[3],), device_id_type=MESH)

    def relay_wait(i):
        ref = YB.at[pl.ds(pl.multiple_of(me * (REGC * 4) + (i + 1) * CHC, 8), CHC)]
        pltpu.make_async_remote_copy(
            src_ref=ref, dst_ref=ref, send_sem=ssem.at[1], recv_sem=rsem.at[i],
            device_id=(peers[1],), device_id_type=MESH).wait_recv()

    ctot = [None] + [slen(peers[k], me) for k in range(1, NDEV)]

    def c_avail(k):
        wp = st[ST_WP + peers[k]]
        return jnp.where(wp == ctot[k], nchunks(wp, CC_SH), wp >> CC_SH)

    cfull = [None] + [ctot[k] >> CC_SH for k in range(1, NDEV)]

    def pump(mode):
        avail = [None] + [c_avail(k) for k in range(1, NDEV)]
        lim = [None] + [jnp.minimum(avail[k], cfull[k]) for k in range(1, NDEV)]
        nr_in, nr_out, ne_o = st[ST_X + 8], st[ST_NR + me], st[ST_NE + me]
        if mode < 2:
            for k in order:
                @pl.when((avail[k] > cfull[k]) & (st[ST_PS + k] == 0))
                def _():
                    partial(ctot[k], KC, lambda n: c_send(k, cfull[k], n).start())
                    st[ST_PS + k] = 1

        if mode == 0:
            nrel = lax.div(jnp.minimum(lim[2], ne_o) * nr_out, jnp.maximum(ne_o, 1))

            def rl(i, _):
                relay1(lst[i], i).start()
                return 0

            lax.fori_loop(st[ST_X + 0], nrel, rl, 0)
            st[ST_X + 0] = nrel
        else:
            nrel = nr_out

        aeff, beff, n_ae = st[ST_X + 2], st[ST_X + 3], st[ST_X + 7]
        rich = st[ST_X + 9] == 1
        err, ca, y0 = st[ST_X + 4], st[ST_CS + 3], st[ST_CS + 2]
        yend = lim[2] - nrel
        ri0 = st[ST_X + 6]
        e1 = jnp.maximum(jnp.minimum(lim[3], n_ae) - ca, 0)
        if mode == 0:
            nr, fa = 0, jnp.maximum(jnp.minimum(lim[3], st[ST_X + 1]) - ca, 0)
            yend = jnp.minimum(yend, st[ST_X + 5])
        elif mode == 1:
            defer = (ri0 < nr_in) | (st[ST_X + 10] == 1)
            yend = jnp.where(defer, y0, yend)
            nr, fa = 0, jnp.where(defer, 0, lim[3] - ca)
        elif mode == 2:
            e1 = jnp.maximum(jnp.minimum(lim[3], st[ST_X + 1]) - ca, 0)
            nr = (nr_in * MID) >> 4
            fa = e1 + nr
        else:
            nr = nr_in - ri0
            fa = lim[3] - ca + nr
        all_b = lim[2] >= (cfull[2] if mode == 1 else ne_o)
        room = (yend - y0) * aeff - err
        xmax = jnp.where(room >= 0, lax.div(jnp.maximum(room, 0), beff) + 1, 0)
        nx = jnp.where(rich | all_b, fa, jnp.minimum(fa, xmax))

        def issue_b(y):
            early = y < ne_o - nr_out
            c = jnp.where(early, lst[NLIST + jnp.where(early, y, 0)], y + nr_out)
            c_send(2, c, CHC).start()

        def bb(y, _):
            issue_b(y)
            return 0

        y1 = jnp.minimum(yend, y0 + lax.div(jnp.maximum(err, 0) + aeff - 1, aeff))
        lax.fori_loop(y0, y1, bb, 0)
        err = err - (y1 - y0) * aeff

        def ab(t, carry):
            err, y = carry
            if mode >= 2:
                is_r = (t >= e1) & (t < e1 + nr)

                @pl.when(is_r)
                def _():
                    ri = ri0 + t - e1
                    relay_wait(ri)
                    relay2(lst[2 * NLIST + ri], ri).start()

                @pl.when(jnp.logical_not(is_r))
                def _():
                    c_send(3, ca + jnp.where(t >= e1, t - nr, t), CHC).start()
            else:
                c_send(3, ca + t, CHC).start()
            err = err + beff
            do_b = (err > 0) & (y < yend)

            @pl.when(do_b)
            def _():
                issue_b(y)

            ib = do_b.astype(jnp.int32)
            return err - ib * aeff, y + ib

        err, y = lax.fori_loop(0, nx, ab, (err, y1))
        y2 = yend if mode == 3 else y if mode == 2 else jnp.where(rich, yend, y)
        lax.fori_loop(y, y2, bb, 0)
        st[ST_X + 4] = jnp.where(rich, 0, err)
        st[ST_CS + 3] = ca + nx - nr
        st[ST_X + 6] = ri0 + nr
        st[ST_CS + 2] = y2

        if mode < 2:
            def yb(c, _):
                c_send(1, c, CHC).start()
                return 0

            lax.fori_loop(st[ST_CS + 1], lim[1], yb, 0)
            st[ST_CS + 1] = lim[1]

    def copy_results(j, s, row_a, row_b):
        e = me * EL + j
        z0 = T(s * ROWS + row_a, e)
        n = T(s * ROWS + row_b, e) - z0
        wp = st[ST_WP + s]
        reg = jnp.where(s == me, NDEV + me, s)
        src0 = (j * ZROWS + z0) * 4
        dst0 = (reg * REGC + wp) * 4

        def cb(i, _):
            YB[pl.ds(dst0 + i * 64, 64), :] = Z[pl.ds(src0 + i * 64, 64), :]
            return 0

        lax.fori_loop(0, (n + 15) >> 4, cb, 0)
        st[ST_WP + s] = wp + n

    def expert(it, _):
        j = jnp.maximum(it - 1, 0)
        e = me * EL + j
        whole = (it >= 2) | jnp.logical_not(light)
        act = [whole | ((it == 0) == (peers[3] == s)) for s in range(NDEV)]

        def fetch(s, g):
            ra, rb = (0, SR) if g == 0 else (SR, ROWS)
            z0 = T(s * ROWS + ra, e)
            n = T(s * ROWS + rb, e) - z0
            p = st[ST_DP + s * 2 + g]
            end = p + dlen(s, g, e)
            st[ST_DP + s * 2 + g] = end

            @pl.when(s != me)
            def _():
                tot_ = dlen(s, g, NE + me)
                need = jnp.minimum(nchunks(end + OVER, CD_SH), nchunks(tot_, CD_SH))
                advance(ST_DW + s * 2 + g, need, tot_, KD,
                        lambda c, ns: d_recv(s, g, c, ns).wait_recv())

            src0 = ((NDEV + s) * REGD + DOFF[g] + p) * 2
            dst0 = z0 * 2
            nbig = n >> 4

            def cb(i, _):
                L[pl.ds(dst0 + i * 32, 32), :] = XB[pl.ds(src0 + i * 32, 32), :]
                return 0

            def cs(i, _):
                L[pl.ds(dst0 + i * 8, 8), :] = XB[pl.ds(src0 + i * 8, 8), :]
                return 0

            lax.fori_loop(0, nbig, cb, 0)
            lax.fori_loop(nbig * 4, (n + 3) >> 2, cs, 0)

        with _scope("assemble"):
            for s in range(NDEV):
                @pl.when(act[s])
                def _():
                    fetch(s, 0)
                    fetch(s, 1)

        @pl.when(whole | (it == 0))
        def _():
            with _scope("wwait"):
                w_cp(j).wait()

        with _scope("matmul"):
            v0 = L[pl.ds(0, MROWS, stride=2), :]
            v1 = L[pl.ds(1, MROWS, stride=2), :]
            lhs = jnp.concatenate(
                [_bf(_unpack_lo(v0)), _bf(_unpack_lo(v1)),
                 _bf(_unpack_hi(v0)), _bf(_unpack_hi(v1))], axis=1)
            zb = j * (ZROWS * 4)
            for n in range(4):
                w = jnp.concatenate(
                    [_bf(wf[j, :, n * 128:(n + 1) * 128]),
                     _bf(wf[j, :, 512 + n * 128:512 + (n + 1) * 128])], axis=1)
                res = _dot(lhs, w)
                Z[pl.ds(zb + n, MROWS, stride=4), :] = _pack(res[:, :128], res[:, 128:])

        @pl.when(j < A_EARLY)
        def _():
            with _scope("early"):
                for s in range(NDEV):
                    @pl.when(act[s])
                    def _():
                        copy_results(j, s, 0, ROWS)

                @pl.when(it == 0)
                def _():
                    n0 = st[ST_WP + peers[3]] >> CC_SH

                    def ab(c, _):
                        c_send(3, c, CHC).start()
                        return 0

                    lax.fori_loop(0, n0, ab, 0)
                    st[ST_CS + 3] = n0
                    free = jnp.maximum(n0 - CREDIT, 0)
                    st[ST_X + 4] = (n0 - free) * st[ST_X + 3]
                    st[ST_X + 2] = jnp.maximum(st[ST_X + 2] - free, st[ST_X + 3])

                @pl.when(it > 0)
                def _():
                    pump(0)

        return 0

    lax.fori_loop(jnp.where(light, 0, 1), EL + 1, expert, 0)

    NCG = len(CGROUPS) - 1
    with _scope("mid"):
        @pl.when(st[ST_X + 8] > 0)
        def _():
            lists(me ^ 1, 2 * NLIST, 3 * NLIST)
            pump(2)

    with _scope("late"):
        set_ratio(cfull[3] - st[ST_CS + 3] + st[ST_X + 8] - st[ST_X + 6] - pick(TAIL_A),
                  cfull[2] - st[ST_NR + me] - st[ST_CS + 2] - pick(TAIL_B))

        def lateg(g, _):
            ra, rb_ = st[ST_CG + g], st[ST_CG + g + 1]
            for j in range(A_EARLY, EL):
                for s in range(NDEV):
                    copy_results(j, s, ra, rb_)
            pump(1)
            return 0

        lax.fori_loop(0, NCG, lateg, 0)
    with _scope("final"):
        pump(3)

    with _scope("drain0"):
        c_cp.wait()
        for k in range(1, NDEV):
            cnt_cp(k).wait_send()
            for g in range(2):
                tot_ = dlen(me, g, NE + peers[k])
                st[ST_SW] = 0
                advance(ST_SW, nchunks(tot_, CD_SH), tot_, KD,
                        lambda c, ns, k=k, g=g: d_send(k, g, c, ns).wait_send())

    def needs(g, _):
        rb_ = st[ST_CG + g + 1]
        for k in range(1, NDEV):
            dev = peers[k]
            endp = slen(me, dev) - (T(me * ROWS + ROWS, NE + NDEV + dev)
                                    - T(me * ROWS + rb_, NE + NDEV + dev))
            need, nfull = nchunks(endp, CC_SH), slen(me, dev) >> CC_SH
            st[ST_ND + 4 + g * 4 + k] = jnp.minimum(need, nfull)
            st[ST_PG + k] = jnp.where(need > nfull, jnp.minimum(st[ST_PG + k], g),
                                      st[ST_PG + k])
        return 0

    for k in range(1, NDEV):
        st[ST_PG + k] = NCG
    lax.fori_loop(0, NCG, needs, 0)
    nsend = (ctot[1] >> CC_SH) + (ctot[2] >> CC_SH) + (ctot[3] >> CC_SH) + st[ST_X + 8]
    for g in range(NCG):
        st[ST_ND + 4 + g * 4] = (nsend * DRAIN[g]) >> 8
    for k in range(NDEV):
        st[ST_ND + k] = 0

    def retire(lo, hi):
        def wb(i, _):
            c_send(1, 0, CHC).wait_send()
            return 0

        lax.fori_loop(lo, hi, wb, 0)

    def outg(g, _):
        ra, rb_ = st[ST_CG + g], st[ST_CG + g + 1]
        with _scope("retire"):
            retire(st[ST_ND + g * 4], st[ST_ND + 4 + g * 4])
        for k in range(1, NDEV):
            with _scope("cw%d" % k):
                def wb(c, _, k=k):
                    c_recv(k, c, CHC).wait_recv()
                    return 0

                lax.fori_loop(st[ST_ND + g * 4 + k], st[ST_ND + 4 + g * 4 + k], wb, 0)

                @pl.when(st[ST_PG + k] == g)
                def _(k=k):
                    rtot = slen(me, peers[k])
                    partial(rtot, KC, lambda n: c_recv(k, rtot >> CC_SH, n).wait_recv())
        with _scope("gather"):
            def gb(row, _):
                base = row * 1024
                for k in range(128):
                    s = slots[ROWS + row, k]
                    v = YB[pl.ds(s, 4), :]
                    o0 = base + (k // 8) * 64 + (k % 8)
                    o_ref[pl.ds(o0, 4, stride=8), :] = _unpack_lo(v)
                    o_ref[pl.ds(o0 + 32, 4, stride=8), :] = _unpack_hi(v)
                return 0

            lax.fori_loop(ra, rb_, gb, 0)
        return 0

    lax.fori_loop(0, NCG, outg, 0)
    with _scope("drain"):
        retire(st[ST_ND + NCG * 4], nsend)
        for k in range(1, NDEV):
            partial(ctot[k], KC, lambda n, k=k: c_send(k, 0, n).wait_send())


def _compiler_params():
    kw = dict(collective_id=0, vmem_limit_bytes=100 * 1024 * 1024)
    try:
        return pltpu.CompilerParams(disable_semaphore_checks=True,
                                    disable_bounds_checks=True, **kw)
    except TypeError:
        return pltpu.CompilerParams(**kw)


def pallas_dist_moe_cap_ep_tokshard_n2048_d512_e8_h1024_kernel(
    x: jax.Array,
    router_W: jax.Array,
    route_idx: jax.Array,
    expert_W: jax.Array,
):
    del router_W
    route = route_idx.astype(jnp.int32).reshape(ROWS, 128)
    u32, f32, i32 = jnp.uint32, jnp.float32, jnp.int32
    scratch = [
        pltpu.VMEM((NT, D), f32),
        pltpu.VMEM((ROWS, 128), i32),
        pltpu.VMEM((EL, D, H), f32),
        pltpu.VMEM((NDEV * ROWS, 128), f32),
        pltpu.VMEM((TROWS, 128), i32),
        pltpu.VMEM((8, 128), i32),
        pltpu.VMEM((2 * ROWS, 128), i32),
        pltpu.VMEM((2 * NT, 128), u32),
        pltpu.VMEM((2 * NDEV * REGD * 2, 128), u32),
        pltpu.VMEM(((MROWS + 16) * 2, 128), u32),
        pltpu.VMEM((EL * ZROWS * 4, 128), u32),
        pltpu.VMEM((2 * NDEV * REGC * 4, 128), u32),
        pltpu.SMEM((TROWS, 128), i32),
        pltpu.SMEM((8, 128), i32),
        pltpu.SMEM((2 * ROWS, 128), i32),
        pltpu.SMEM((160,), i32),
        pltpu.SMEM((4 * NLIST,), i32),
        pltpu.SemaphoreType.DMA((32,)),
        pltpu.SemaphoreType.DMA((6,)),
        pltpu.SemaphoreType.DMA((NDSEM,)),
        pltpu.SemaphoreType.DMA((NCSEM,)),
        pltpu.SemaphoreType.DMA((NRELAY,)),
        pltpu.SemaphoreType.DMA((2,)),
    ]
    out = pl.pallas_call(
        _body,
        out_shape=jax.ShapeDtypeStruct((NT * 8, 128), f32),
        in_specs=[pl.BlockSpec(memory_space=pl.ANY)] * 3,
        out_specs=pl.BlockSpec(memory_space=pltpu.VMEM),
        scratch_shapes=scratch,
        compiler_params=_compiler_params(),
    )(x, route, expert_W)
    return out.reshape(NT // 8, 8, 8, 128).transpose(0, 2, 1, 3).reshape(NT, H)
```
